```python
import numpy as np

kernel_name = "dist_mean_ax0_shard0_i_m4096_n1024"

def setup_inputs():
    return {"x": np.random.randn(16384, 1024).astype(np.float32)}

def reference(x: np.ndarray) -> np.ndarray:
    return np.mean(x, axis=0, keepdims=True)
```

```python
import jax
import jax.numpy as jnp
from jax import lax
from jax.experimental import pallas as pl
from jax.experimental.pallas import tpu as pltpu

N_DEV = 4
SIDE_ROWS = 208
MID_ROWS = 64
TAIL_ROWS = 384
TAIL_COLS = 128
UNROLL = 64


def _accum(ref, start, rows, acc, c0, w):
    full = rows // UNROLL

    def group(r0, r):
        blk = ref[pl.ds(r0, r), pl.ds(c0, w)]
        return jnp.sum(blk.reshape(r // 8, 8, w), axis=0)

    if full > 1:
        acc = lax.fori_loop(
            0, full,
            lambda i, a: a + group(pl.multiple_of(start + i * UNROLL, 8), UNROLL),
            acc)
    elif full == 1:
        acc = acc + group(start, UNROLL)
    rem = rows - full * UNROLL
    if rem:
        acc = acc + group(start + full * UNROLL, rem)
    return acc


def _tree_sum(vs):
    while len(vs) > 1:
        nxt = [vs[i] + vs[i + 1] for i in range(0, len(vs) - 1, 2)]
        if len(vs) % 2:
            nxt.append(vs[-1])
        vs = nxt
    return vs[0]


def pallas_dist_mean_ax0_shard0_i_m4096_n1024_kernel(x: jax.Array):
    m, n = x.shape
    inv = 1.0 / (m * N_DEV)
    w1 = n - TAIL_COLS
    local_rows = m - 2 * SIDE_ROWS
    tail0 = local_rows - TAIL_ROWS
    big = tail0 - MID_ROWS
    pieces = [
        (0, big, 0, n),
        (tail0, TAIL_ROWS, 0, w1),
        (big, MID_ROWS, 0, n),
        (tail0, TAIL_ROWS, w1, TAIL_COLS),
    ]

    def body(x_hbm, out_ref, buf, side_buf, s1, s2, r1, r2,
             load_sems, side_send, side_recv, send_sems, recv_sems):
        me = lax.axis_index("i")

        def peer(d):
            return ((me + d) % N_DEV,)

        def load(i):
            r0, rows, c0, cols = pieces[i]
            return pltpu.make_async_copy(
                x_hbm.at[pl.ds(r0, rows), pl.ds(c0, cols)],
                buf.at[pl.ds(r0, rows), pl.ds(c0, cols)],
                load_sems.at[i])

        def side(k):
            return pltpu.make_async_remote_copy(
                src_ref=x_hbm.at[pl.ds(local_rows + k * SIDE_ROWS, SIDE_ROWS), :],
                dst_ref=side_buf.at[k],
                send_sem=side_send.at[k], recv_sem=side_recv.at[k],
                device_id=peer((1, 3)[k]), device_id_type=pl.DeviceIdType.MESH)

        def share(which, d):
            s, r = ((s1, r1), (s2, r2))[which]
            j = which * (N_DEV - 1) + d - 1
            return pltpu.make_async_remote_copy(
                src_ref=s, dst_ref=r.at[d - 1],
                send_sem=send_sems.at[j], recv_sem=recv_sems.at[j],
                device_id=peer(d), device_id_type=pl.DeviceIdType.MESH)

        for i in range(len(pieces)):
            load(i).start()

        barrier = pltpu.get_barrier_semaphore()
        for d in range(1, N_DEV):
            pl.semaphore_signal(barrier, inc=1, device_id=peer(d),
                                device_id_type=pl.DeviceIdType.MESH)
        pl.semaphore_wait(barrier, N_DEV - 1)

        for k in range(2):
            side(k).start()

        load(0).wait()
        acc = _accum(buf, 0, big, jnp.zeros((8, n), jnp.float32), 0, n)
        load(1).wait()
        acc_b = _accum(buf, tail0, TAIL_ROWS, jnp.zeros((8, w1), jnp.float32), 0, w1)
        for k in range(2):
            side(k).wait_recv()
            acc = _accum(side_buf.at[k], 0, SIDE_ROWS, acc, 0, n)
        load(2).wait()
        acc = _accum(buf, big, MID_ROWS, acc, 0, n)
        s1[...] = jnp.sum(acc[:, :w1] + acc_b, axis=0, keepdims=True) * inv
        for d in (2, 1, 3):
            share(0, d).start()

        load(3).wait()
        acc_c = acc[:, w1:] + _tree_sum(
            [buf[pl.ds(tail0 + 8 * i, 8), pl.ds(w1, TAIL_COLS)]
             for i in range(TAIL_ROWS // 8)])
        s2[...] = jnp.sum(acc_c, axis=0, keepdims=True) * inv
        for d in (2, 1, 3):
            share(1, d).start()

        for k in range(2):
            side(k).wait_send()
        for which in range(2):
            for d in range(1, N_DEV):
                share(which, d).wait_send()
        for which in range(2):
            share(which, 1).wait_recv()
            share(which, 3).wait_recv()
        t1 = s1[...] + r1[0] + r1[2]
        t2 = s2[...] + r2[0] + r2[2]
        share(0, 2).wait_recv()
        out_ref[:, pl.ds(0, w1)] = t1 + r1[1]
        share(1, 2).wait_recv()
        out_ref[:, pl.ds(w1, TAIL_COLS)] = t2 + r2[1]

    return pl.pallas_call(
        body,
        out_shape=jax.ShapeDtypeStruct((1, n), jnp.float32),
        in_specs=[pl.BlockSpec(memory_space=pl.ANY)],
        out_specs=pl.BlockSpec(memory_space=pltpu.VMEM),
        scratch_shapes=[
            pltpu.VMEM((local_rows, n), jnp.float32),
            pltpu.VMEM((2, SIDE_ROWS, n), jnp.float32),
            pltpu.VMEM((1, w1), jnp.float32),
            pltpu.VMEM((1, TAIL_COLS), jnp.float32),
            pltpu.VMEM((N_DEV - 1, 1, w1), jnp.float32),
            pltpu.VMEM((N_DEV - 1, 1, TAIL_COLS), jnp.float32),
            pltpu.SemaphoreType.DMA((len(pieces),)),
            pltpu.SemaphoreType.DMA((2,)),
            pltpu.SemaphoreType.DMA((2,)),
            pltpu.SemaphoreType.DMA((2 * (N_DEV - 1),)),
            pltpu.SemaphoreType.DMA((2 * (N_DEV - 1),)),
        ],
        compiler_params=pltpu.CompilerParams(
            collective_id=0,
            vmem_limit_bytes=64 * 1024 * 1024,
            disable_semaphore_checks=True,
        ),
    )(x)
```

```python
import jax
import jax.numpy as jnp
from jax import lax
from jax.experimental import pallas as pl
from jax.experimental.pallas import tpu as pltpu

N_DEV = 4
N_REG = 8
HALF = N_REG // 2
LEAD = 8
LAG = 10
TAIL_COLS = 128
LATE_STEPS = 2


def _tree_sum(vs):
    while len(vs) > 1:
        nxt = [vs[i] + vs[i + 1] for i in range(0, len(vs) - 1, 2)]
        if len(vs) % 2:
            nxt.append(vs[-1])
        vs = nxt
    return vs[0]


def _compiler_params():
    base = dict(collective_id=0, vmem_limit_bytes=64 * 1024 * 1024)
    try:
        return pltpu.CompilerParams(disable_semaphore_checks=True, **base)
    except TypeError:
        return pltpu.CompilerParams(**base)


def pallas_dist_mean_ax0_shard0_i_m4096_n1024_kernel(x: jax.Array):
    m, n = x.shape
    steps = m // (8 * N_REG)
    reg_rows = steps * 8
    assert reg_rows * N_REG == m
    inv = 1.0 / (m * N_DEV)
    w1 = n - TAIL_COLS
    tail_rows = reg_rows // (LEAD * HALF)
    assert tail_rows * LEAD * HALF == reg_rows and tail_rows % 8 == 0
    early_rows = (LEAD - LATE_STEPS) * HALF * tail_rows

    def body(x_hbm, out_ref, buf, buf_head, buf_tail, s1, s2, r1, r2,
             sem, sem_head, sem_tail, send_sems, recv_sems):
        me = lax.axis_index("i")

        def peer(d):
            return ((me + d) % N_DEV,)

        def rows(region, t):
            return pl.ds(pl.multiple_of(region * reg_rows + t * 8, 8), 8)

        def start_hi(t, u):
            pltpu.make_async_copy(
                x_hbm.at[rows(HALF + u, t), :],
                buf.at[t, pl.ds(u * 8, 8), :],
                sem.at[t]).start(priority=0)

        def start_lo(t, u):
            if u < HALF - 1:
                pltpu.make_async_copy(
                    x_hbm.at[rows(u + 1, t), :],
                    buf.at[t, pl.ds((HALF + u) * 8, 8), :],
                    sem.at[t]).start(priority=1)
            else:
                pltpu.make_async_copy(
                    x_hbm.at[rows(0, t), pl.ds(0, w1)],
                    buf_head.at[t],
                    sem_head.at[t]).start(priority=1)

        def start_tail(j, which):
            r = pl.ds(pl.multiple_of(j * tail_rows, 8), tail_rows)
            pltpu.make_async_copy(
                x_hbm.at[r, pl.ds(w1, TAIL_COLS)],
                buf_tail.at[r, :],
                sem_tail.at[which]).start(priority=1)

        def wait_filled(ref, s):
            pltpu.make_async_copy(ref, ref, s).wait()

        def consume(t, acc):
            a1, a2 = acc
            wait_filled(buf_head.at[t], sem_head.at[t])
            wait_filled(buf.at[t], sem.at[t])
            v = jnp.sum(buf[t].reshape(N_REG - 1, 8, n), axis=0)
            return a1 + (v[:, :w1] + buf_head[t]), a2 + v[:, w1:]

        def lead_in(t, carry):
            for u in range(HALF):
                start_lo(t, u)
            return carry

        def phase(lo, hi, acc, tail=None, cons=True):
            def step(s, acc):
                for u in range(HALF):
                    start_hi(s, u)
                    if tail is None:
                        start_lo(s + LEAD, u)
                    else:
                        start_tail((s - (steps - LEAD)) * HALF + u, tail)
                return consume(s - LAG, acc) if cons else acc
            return lax.fori_loop(lo, hi, step, acc)

        lax.fori_loop(0, LEAD, lead_in, 0)

        barrier = pltpu.get_barrier_semaphore()
        for d in range(1, N_DEV):
            pl.semaphore_signal(barrier, inc=1, device_id=peer(d),
                                device_id_type=pl.DeviceIdType.MESH)

        phase(0, LAG, 0, cons=False)
        acc = (jnp.zeros((8, w1), jnp.float32),
               jnp.zeros((8, TAIL_COLS), jnp.float32))
        acc = phase(LAG, steps - LEAD, acc)
        acc = phase(steps - LEAD, steps - LATE_STEPS, acc, tail=0)
        acc = phase(steps - LATE_STEPS, steps, acc, tail=1)
        pl.semaphore_wait(barrier, N_DEV - 1)
        a1, a2 = lax.fori_loop(steps - LAG, steps, consume, acc)

        def share(which, d):
            s, r = ((s1, r1), (s2, r2))[which]
            j = which * (N_DEV - 1) + d - 1
            return pltpu.make_async_remote_copy(
                src_ref=s, dst_ref=r.at[d - 1],
                send_sem=send_sems.at[j], recv_sem=recv_sems.at[j],
                device_id=peer(d), device_id_type=pl.DeviceIdType.MESH)

        s1[...] = jnp.sum(a1, axis=0, keepdims=True) * inv
        for d in (2, 1, 3):
            share(0, d).start()

        for which, (r0, r1_) in enumerate(((0, early_rows), (early_rows, reg_rows))):
            wait_filled(buf_tail.at[pl.ds(r0, r1_ - r0), :], sem_tail.at[which])
            a2 = a2 + _tree_sum(
                [buf_tail[pl.ds(r, 8), :] for r in range(r0, r1_, 8)])
        s2[...] = jnp.sum(a2, axis=0, keepdims=True) * inv
        for d in (2, 1, 3):
            share(1, d).start()

        for which in range(2):
            for d in range(1, N_DEV):
                share(which, d).wait_send()
        for which in range(2):
            share(which, 1).wait_recv()
            share(which, 3).wait_recv()
        t1 = s1[...] + r1[0] + r1[2]
        t2 = s2[...] + r2[0] + r2[2]
        share(0, 2).wait_recv()
        out_ref[:, pl.ds(0, w1)] = t1 + r1[1]
        share(1, 2).wait_recv()
        out_ref[:, pl.ds(w1, TAIL_COLS)] = t2 + r2[1]

    return pl.pallas_call(
        body,
        out_shape=jax.ShapeDtypeStruct((1, n), jnp.float32),
        in_specs=[pl.BlockSpec(memory_space=pl.ANY)],
        out_specs=pl.BlockSpec(memory_space=pltpu.VMEM),
        scratch_shapes=[
            pltpu.VMEM((steps, (N_REG - 1) * 8, n), jnp.float32),
            pltpu.VMEM((steps, 8, w1), jnp.float32),
            pltpu.VMEM((reg_rows, TAIL_COLS), jnp.float32),
            pltpu.VMEM((1, w1), jnp.float32),
            pltpu.VMEM((1, TAIL_COLS), jnp.float32),
            pltpu.VMEM((N_DEV - 1, 1, w1), jnp.float32),
            pltpu.VMEM((N_DEV - 1, 1, TAIL_COLS), jnp.float32),
            pltpu.SemaphoreType.DMA((steps,)),
            pltpu.SemaphoreType.DMA((steps,)),
            pltpu.SemaphoreType.DMA((2,)),
            pltpu.SemaphoreType.DMA((2 * (N_DEV - 1),)),
            pltpu.SemaphoreType.DMA((2 * (N_DEV - 1),)),
        ],
        compiler_params=_compiler_params(),
    )(x)
```

```python
import jax
import jax.numpy as jnp
from jax import lax
from jax.experimental import pallas as pl
from jax.experimental.pallas import tpu as pltpu

N_DEV = 4
N_REG = 8
HALF = N_REG // 2
LEAD = 4
LAG = 5


def _tree_sum(vs):
    while len(vs) > 1:
        nxt = [vs[i] + vs[i + 1] for i in range(0, len(vs) - 1, 2)]
        if len(vs) % 2:
            nxt.append(vs[-1])
        vs = nxt
    return vs[0]


def _compiler_params():
    base = dict(collective_id=0, vmem_limit_bytes=64 * 1024 * 1024)
    try:
        return pltpu.CompilerParams(disable_semaphore_checks=True, **base)
    except TypeError:
        return pltpu.CompilerParams(**base)


def pallas_dist_mean_ax0_shard0_i_m4096_n1024_kernel(x: jax.Array):
    m, n = x.shape
    cb = n // 128
    groups = m // 8
    tiles = groups * cb
    reg = tiles // N_REG
    unit = 2 * cb
    steps = reg // unit
    head = cb - 1
    w1 = head * 128
    inv = 1.0 / (m * N_DEV)
    assert cb == 8 and steps * unit * N_REG == tiles
    assert steps == LEAD * N_REG

    def body(x4_hbm, out_ref, buf, s1, s2, r1, r2, sems, send_sems, recv_sems):
        x_hbm = x4_hbm.reshape(tiles, 8, 128)

        def slot(hi, u, j):
            return (u // 2) * 8 + (0 if hi else 4) + 2 * (u % 2) + j

        def sem(kind, t):
            return sems.at[kind * steps + t]

        def first_tile(region, t, j):
            return region * reg + head + j * cb + t * unit

        def start_hi(t, u, j, wrap=False):
            dst, s = buf.at[t, slot(True, u, j)], sem(u // 2, t)
            if wrap:
                pltpu.make_async_copy(x_hbm.at[pl.ds(tiles - 1, 1)],
                                      dst.at[pl.ds(0, 1)], s).start(priority=0)
                pltpu.make_async_copy(x_hbm.at[pl.ds(0, head)],
                                      dst.at[pl.ds(1, head)], s).start(priority=0)
            else:
                pltpu.make_async_copy(
                    x_hbm.at[pl.ds(first_tile(HALF + u, t, j), cb)],
                    dst, s).start(priority=0)

        def start_lo(t, u, j):
            dst = buf.at[t, slot(False, u, j)]
            if u < HALF - 1:
                pltpu.make_async_copy(
                    x_hbm.at[pl.ds(first_tile(u + 1, t, j), cb)],
                    dst, sem(u // 2, t)).start(priority=1)
            else:
                pltpu.make_async_copy(
                    x_hbm.at[pl.ds(first_tile(0, t, j) + 1, head)],
                    dst.at[pl.ds(1, head)], sem(2, t)).start(priority=1)

        def start_tail(w, q, which):
            pltpu.make_async_copy(
                x4_hbm.at[pl.ds(2 * (w * N_REG + q), 2), head],
                buf.at[steps, 2 * w + q // 4, pl.ds(2 * (q % 4), 2)],
                sem(3, which)).start(priority=1)

        def wait_filled(ref, s):
            pltpu.make_async_copy(ref, ref, s).wait()

        def consume(t, acc):
            a1, a2 = acc
            wait_filled(buf.at[t, pl.ds(0, 8)], sem(0, t))
            v = jnp.sum(buf[t, pl.ds(0, 8)], axis=0)
            a1, a2 = a1 + v[1:], a2 + v[0]
            wait_filled(buf.at[t, pl.ds(14, 2), pl.ds(1, head)], sem(2, t))
            wait_filled(buf.at[t, pl.ds(8, 6)], sem(1, t))
            v = jnp.sum(buf[t, pl.ds(8, 6)], axis=0)
            h = buf[t, 14, pl.ds(1, head)] + buf[t, 15, pl.ds(1, head)]
            return a1 + (v[1:] + h), a2 + v[0]

        def lead_in(t, carry):
            for u in range(HALF):
                for j in range(2):
                    start_lo(t, u, j)
            return carry

        def issue(s, tail=None, last=False):
            for u in range(HALF):
                for j in range(2):
                    start_hi(s, u, j, wrap=last and (u, j) == (HALF - 1, 1))
                    if tail is None:
                        start_lo(s + LEAD, u, j)
                    else:
                        start_tail(s - (steps - LEAD), 2 * u + j, tail)

        def phase(lo, hi, acc, tail=None, cons=True):
            def step(s, acc):
                issue(s, tail)
                return consume(s - LAG, acc) if cons else acc
            return lax.fori_loop(lo, hi, step, acc)

        lax.fori_loop(0, LEAD, lead_in, 0)

        me = lax.axis_index("i")

        def peer(d):
            return ((me + d) % N_DEV,)

        barrier = pltpu.get_barrier_semaphore()
        for d in range(1, N_DEV):
            pl.semaphore_signal(barrier, inc=1, device_id=peer(d),
                                device_id_type=pl.DeviceIdType.MESH)

        phase(0, LAG, 0, cons=False)
        acc = (jnp.zeros((head, 8, 128), jnp.float32),
               jnp.zeros((8, 128), jnp.float32))
        acc = phase(LAG, steps - LEAD, acc)
        acc = phase(steps - LEAD, steps - 1, acc, tail=0)
        issue(steps - 1, tail=1, last=True)
        pl.semaphore_wait(barrier, N_DEV - 1)
        a1, a2 = lax.fori_loop(steps - 1 - LAG, steps, consume, acc)

        def share(which, d):
            s, r = ((s1, r1), (s2, r2))[which]
            j = which * (N_DEV - 1) + d - 1
            return pltpu.make_async_remote_copy(
                src_ref=s, dst_ref=r.at[d - 1],
                send_sem=send_sems.at[j], recv_sem=recv_sems.at[j],
                device_id=peer(d), device_id_type=pl.DeviceIdType.MESH)

        s1[...] = jnp.concatenate(
            [jnp.sum(a1[c], axis=0, keepdims=True) for c in range(head)],
            axis=1) * inv
        for d in (2, 1, 3):
            share(0, d).start()

        early = 2 * (LEAD - 1)
        for which, (k0, k1) in enumerate(((0, early), (early, 2 * LEAD))):
            wait_filled(buf.at[steps, pl.ds(k0, k1 - k0)], sem(3, which))
            a2 = a2 + _tree_sum(
                [buf[steps, k, j] for k in range(k0, k1) for j in range(cb)])
        s2[...] = jnp.sum(a2, axis=0, keepdims=True) * inv
        for d in (2, 1, 3):
            share(1, d).start()

        for which in range(2):
            for d in range(1, N_DEV):
                share(which, d).wait_send()
        for which in range(2):
            share(which, 1).wait_recv()
            share(which, 3).wait_recv()
        t1 = s1[...] + r1[0] + r1[2]
        t2 = s2[...] + r2[0] + r2[2]
        share(0, 2).wait_recv()
        out_ref[:, pl.ds(0, w1)] = t1 + r1[1]
        share(1, 2).wait_recv()
        out_ref[:, pl.ds(w1, 128)] = t2 + r2[1]

    x4 = x.reshape(groups, 8, cb, 128).transpose(0, 2, 1, 3)
    return pl.pallas_call(
        body,
        out_shape=jax.ShapeDtypeStruct((1, n), jnp.float32),
        in_specs=[pl.BlockSpec(memory_space=pl.ANY)],
        out_specs=pl.BlockSpec(memory_space=pltpu.VMEM),
        scratch_shapes=[
            pltpu.VMEM((steps + 1, 2 * N_REG, cb, 8, 128), jnp.float32),
            pltpu.VMEM((1, w1), jnp.float32),
            pltpu.VMEM((1, 128), jnp.float32),
            pltpu.VMEM((N_DEV - 1, 1, w1), jnp.float32),
            pltpu.VMEM((N_DEV - 1, 1, 128), jnp.float32),
            pltpu.SemaphoreType.DMA((3 * steps + 2,)),
            pltpu.SemaphoreType.DMA((2 * (N_DEV - 1),)),
            pltpu.SemaphoreType.DMA((2 * (N_DEV - 1),)),
        ],
        compiler_params=_compiler_params(),
    )(x4)
```

```python
import jax
import jax.numpy as jnp
from jax import lax
from jax.experimental import pallas as pl
from jax.experimental.pallas import tpu as pltpu

N_DEV = 4
N_REG = 8
HALF = N_REG // 2
LEAD = 4
LAG = 5


def _tree_sum(vs):
    while len(vs) > 1:
        nxt = [vs[i] + vs[i + 1] for i in range(0, len(vs) - 1, 2)]
        if len(vs) % 2:
            nxt.append(vs[-1])
        vs = nxt
    return vs[0]


def _compiler_params():
    base = dict(collective_id=0, vmem_limit_bytes=64 * 1024 * 1024)
    try:
        return pltpu.CompilerParams(disable_semaphore_checks=True, **base)
    except TypeError:
        return pltpu.CompilerParams(**base)


def pallas_dist_mean_ax0_shard0_i_m4096_n1024_kernel(x: jax.Array):
    m, n = x.shape
    cb = n // 128
    groups = m // 8
    tiles = groups * cb
    reg = tiles // N_REG
    unit = 2 * cb
    steps = reg // unit
    head = cb - 1
    w1 = head * 128
    inv = 1.0 / (m * N_DEV)
    assert cb == 8 and steps * unit * N_REG == tiles
    assert steps == LEAD * N_REG

    def body(x_hbm, x4_hbm, out_ref, buf, s1, s2, r1, r2,
             sems, send_sems, recv_sems):
        def slot(hi, u, j):
            return (u // 2) * 8 + (0 if hi else 4) + 2 * (u % 2) + j

        def sem(kind, t):
            return sems.at[kind * steps + t]

        def first_tile(region, t, j):
            return region * reg + head + j * cb + t * unit

        def start_hi(t, u, j, wrap=False):
            dst, s = buf.at[t, slot(True, u, j)], sem(u // 2, t)
            if wrap:
                pltpu.make_async_copy(x_hbm.at[pl.ds(tiles - 1, 1)],
                                      dst.at[pl.ds(0, 1)], s).start(priority=0)
                pltpu.make_async_copy(x_hbm.at[pl.ds(0, head)],
                                      dst.at[pl.ds(1, head)], s).start(priority=0)
            else:
                pltpu.make_async_copy(
                    x_hbm.at[pl.ds(first_tile(HALF + u, t, j), cb)],
                    dst, s).start(priority=0)

        def start_lo(t, u, j):
            dst = buf.at[t, slot(False, u, j)]
            if u < HALF - 1:
                pltpu.make_async_copy(
                    x_hbm.at[pl.ds(first_tile(u + 1, t, j), cb)],
                    dst, sem(u // 2, t)).start(priority=1)
            else:
                pltpu.make_async_copy(
                    x_hbm.at[pl.ds(first_tile(0, t, j) + 1, head)],
                    dst.at[pl.ds(1, head)], sem(2, t)).start(priority=1)

        def start_tail(w, q, which):
            pltpu.make_async_copy(
                x4_hbm.at[pl.ds(2 * (w * N_REG + q), 2), head],
                buf.at[steps, 2 * w + q // 4, pl.ds(2 * (q % 4), 2)],
                sem(3, which)).start(priority=1)

        def wait_filled(ref, s):
            pltpu.make_async_copy(ref, ref, s).wait()

        def consume(t, acc):
            a1, a2 = acc
            wait_filled(buf.at[t, pl.ds(0, 8)], sem(0, t))
            v = jnp.sum(buf[t, pl.ds(0, 8)], axis=0)
            a1, a2 = a1 + v[1:], a2 + v[0]
            wait_filled(buf.at[t, pl.ds(14, 2), pl.ds(1, head)], sem(2, t))
            wait_filled(buf.at[t, pl.ds(8, 6)], sem(1, t))
            v = jnp.sum(buf[t, pl.ds(8, 6)], axis=0)
            h = buf[t, 14, pl.ds(1, head)] + buf[t, 15, pl.ds(1, head)]
            return a1 + (v[1:] + h), a2 + v[0]

        def lead_in(t, carry):
            for u in range(HALF):
                for j in range(2):
                    start_lo(t, u, j)
            return carry

        def issue(s, tail=None, last=False):
            for u in range(HALF):
                for j in range(2):
                    start_hi(s, u, j, wrap=last and (u, j) == (HALF - 1, 1))
                    if tail is None:
                        start_lo(s + LEAD, u, j)
                    else:
                        start_tail(s - (steps - LEAD), 2 * u + j, tail)

        def phase(lo, hi, acc, tail=None, cons=True):
            def step(s, acc):
                issue(s, tail)
                return consume(s - LAG, acc) if cons else acc
            return lax.fori_loop(lo, hi, step, acc)

        lax.fori_loop(0, LEAD, lead_in, 0)

        me = lax.axis_index("i")

        def peer(d):
            return ((me + d) % N_DEV,)

        barrier = pltpu.get_barrier_semaphore()
        for d in range(1, N_DEV):
            pl.semaphore_signal(barrier, inc=1, device_id=peer(d),
                                device_id_type=pl.DeviceIdType.MESH)

        phase(0, LAG, 0, cons=False)
        acc = (jnp.zeros((head, 8, 128), jnp.float32),
               jnp.zeros((8, 128), jnp.float32))
        acc = phase(LAG, steps - LEAD, acc)
        acc = phase(steps - LEAD, steps - 1, acc, tail=0)
        issue(steps - 1, tail=1, last=True)
        pl.semaphore_wait(barrier, N_DEV - 1)
        a1, a2 = lax.fori_loop(steps - 1 - LAG, steps, consume, acc)

        def share(which, d):
            s, r = ((s1, r1), (s2, r2))[which]
            j = which * (N_DEV - 1) + d - 1
            return pltpu.make_async_remote_copy(
                src_ref=s, dst_ref=r.at[d - 1],
                send_sem=send_sems.at[j], recv_sem=recv_sems.at[j],
                device_id=peer(d), device_id_type=pl.DeviceIdType.MESH)

        s1[...] = jnp.concatenate(
            [jnp.sum(a1[c], axis=0, keepdims=True) for c in range(head)],
            axis=1) * inv
        for d in (2, 1, 3):
            share(0, d).start()

        early = 2 * (LEAD - 1)
        for which, (k0, k1) in enumerate(((0, early), (early, 2 * LEAD))):
            wait_filled(buf.at[steps, pl.ds(k0, k1 - k0)], sem(3, which))
            a2 = a2 + _tree_sum(
                [buf[steps, k, j] for k in range(k0, k1) for j in range(cb)])
        s2[...] = jnp.sum(a2, axis=0, keepdims=True) * inv
        for d in (2, 1, 3):
            share(1, d).start()

        for which in range(2):
            for d in range(1, N_DEV):
                share(which, d).wait_send()
        for which in range(2):
            share(which, 1).wait_recv()
            share(which, 3).wait_recv()
        t1 = s1[...] + r1[0] + r1[2]
        t2 = s2[...] + r2[0] + r2[2]
        share(0, 2).wait_recv()
        out_ref[:, pl.ds(0, w1)] = t1 + r1[1]
        share(1, 2).wait_recv()
        out_ref[:, pl.ds(w1, 128)] = t2 + r2[1]

    x4 = x.reshape(groups, 8, cb, 128).transpose(0, 2, 1, 3)
    x3 = x4.reshape(tiles, 8, 128)
    return pl.pallas_call(
        body,
        out_shape=jax.ShapeDtypeStruct((1, n), jnp.float32),
        in_specs=[pl.BlockSpec(memory_space=pl.ANY)] * 2,
        out_specs=pl.BlockSpec(memory_space=pltpu.VMEM),
        scratch_shapes=[
            pltpu.VMEM((steps + 1, 2 * N_REG, cb, 8, 128), jnp.float32),
            pltpu.VMEM((1, w1), jnp.float32),
            pltpu.VMEM((1, 128), jnp.float32),
            pltpu.VMEM((N_DEV - 1, 1, w1), jnp.float32),
            pltpu.VMEM((N_DEV - 1, 1, 128), jnp.float32),
            pltpu.SemaphoreType.DMA((3 * steps + 2,)),
            pltpu.SemaphoreType.DMA((2 * (N_DEV - 1),)),
            pltpu.SemaphoreType.DMA((2 * (N_DEV - 1),)),
        ],
        compiler_params=_compiler_params(),
    )(x3, x4)
```
